```python
import numpy as np

kernel_name = "dist_moe_shared_ep_outshard_n256_d128_e2_h256"

def setup_inputs():
    x = np.random.randn(256, 128).astype(np.float32)
    router_W = np.random.randn(128, 8).astype(np.float32) * 0.1
    scores64 = x.astype(np.float64) @ router_W.astype(np.float64)
    route_idx = np.argsort(-scores64, axis=-1)[:, :1].astype(np.int32)
    expert_W = np.random.randn(8, 128, 256).astype(np.float32) * 0.02
    shared_W = np.random.randn(128, 256).astype(np.float32) * 0.02
    return {"x": x, "router_W": router_W, "route_idx": route_idx, "expert_W": expert_W, "shared_W": shared_W}

def reference(x, router_W, route_idx, expert_W, shared_W):
    scores = x @ router_W
    s_max = scores.max(axis=-1, keepdims=True)
    probs = np.exp(scores - s_max)
    probs = probs / probs.sum(axis=-1, keepdims=True)
    shared = x @ shared_W
    out = np.zeros((256, 256), dtype=np.float32)
    for i in range(256):
        e = int(route_idx[i, 0])
        out[i] = shared[i] + probs[i, e] * (x[i] @ expert_W[e])
    return out
```

```python
import jax
import jax.numpy as jnp
from jax import lax
from jax.experimental import pallas as pl
from jax.experimental.pallas import tpu as pltpu

N_DEV = 4
ROWS = 64
D = 128
H = 256
BF = jnp.bfloat16
F32 = jnp.float32

def pallas_dist_moe_shared_ep_outshard_n256_d128_e2_h256_kernel(x, router_W, route_idx, expert_W, shared_W):
    def body(x_hbm, rw_hbm, idx_hbm, ew_hbm, sw_hbm, out_ref,
             x_v, rw_v, idx_v, ew_v, sw_v, icol, send_buf, recv_buf, ld_sems, send_sems, recv_sems):
        me = lax.axis_index("i")
        blk = [(me + k) & 3 for k in range(N_DEV)]
        rows = [pl.ds(pl.multiple_of(b * ROWS, ROWS), ROWS) for b in blk]
        ld_idx = pltpu.make_async_copy(idx_hbm, idx_v, ld_sems.at[0])
        ld_ew = pltpu.make_async_copy(ew_hbm, ew_v, ld_sems.at[1])
        ld_x = [pltpu.make_async_copy(x_hbm.at[rows[k]], x_v.at[k], ld_sems.at[2 + k]) for k in range(N_DEV)]
        ld_rw = pltpu.make_async_copy(rw_hbm, rw_v, ld_sems.at[6])
        ld_sw = pltpu.make_async_copy(sw_hbm, sw_v, ld_sems.at[7])
        ld_idx.start(); ld_x[2].start(); ld_ew.start()
        bar = pltpu.get_barrier_semaphore()
        for k in (2, 1, 3):
            pl.semaphore_signal(bar, inc=1, device_id=(blk[k],), device_id_type=pl.DeviceIdType.MESH)
        ld_x[1].start(); ld_x[3].start(); ld_x[0].start(); ld_rw.start(); ld_sw.start()

        ld_idx.wait()
        e_row = idx_v[...] & 7
        icol[...] = jnp.broadcast_to(e_row, (128, 256)).T
        ld_x[2].wait()
        ld_ew.wait()
        w = ew_v[...].reshape(2 * D, H).astype(BF)

        def contrib(k):
            xb = x_v[k]
            e = icol[rows[k], :]
            lhs = jnp.concatenate([jnp.where(e == 2 * me, xb, 0.0), jnp.where(e == 2 * me + 1, xb, 0.0)], axis=1).astype(BF)
            return jnp.dot(lhs, w, preferred_element_type=F32)

        rdmas = []
        for k in (2, 1, 3):
            if k != 2:
                ld_x[k].wait()
            send_buf[k - 1] = contrib(k).astype(BF)
            if k == 2:
                pl.semaphore_wait(bar, 3)
            r = pltpu.make_async_remote_copy(send_buf.at[k - 1], recv_buf.at[k - 1], send_sems.at[k - 1], recv_sems.at[k - 1],
                                             device_id=(blk[k],), device_id_type=pl.DeviceIdType.MESH)
            r.start()
            rdmas.append(r)
        ld_x[0].wait(); ld_rw.wait(); ld_sw.wait()
        own = contrib(0)
        xm = x_v[0]
        e = icol[rows[0], :]
        scores = lax.dot_general(xm, rw_v[...], (((1,), (1,)), ((), ())), preferred_element_type=F32, precision=lax.Precision.HIGHEST)
        m = jnp.max(scores, axis=-1, keepdims=True)
        pe = jnp.exp(scores - m)
        den = jnp.sum(pe, axis=-1, keepdims=True)
        lane = lax.broadcasted_iota(jnp.int32, scores.shape, 1)
        p = jnp.sum(jnp.where(lane == e[:, :8], pe, 0.0), axis=-1, keepdims=True) / den
        shared = jnp.dot(xm.astype(BF), sw_v[...].astype(BF), preferred_element_type=F32)
        rdmas[1].wait_recv(); rdmas[2].wait_recv()
        base = shared + p * (own + recv_buf[0].astype(F32) + recv_buf[2].astype(F32))
        rdmas[0].wait_recv()
        out_ref[...] = base + p * recv_buf[1].astype(F32)
        for q in rdmas:
            q.wait_send()

    hbm = pl.BlockSpec(memory_space=pltpu.HBM)
    return pl.pallas_call(
        body,
        out_shape=jax.ShapeDtypeStruct((ROWS, H), F32),
        in_specs=[hbm] * 5, out_specs=pl.BlockSpec(memory_space=pltpu.VMEM),
        scratch_shapes=[pltpu.VMEM((N_DEV, ROWS, D), F32), pltpu.VMEM((8, D), F32), pltpu.VMEM((1, 256), jnp.int32),
                        pltpu.VMEM((2, D, H), F32), pltpu.VMEM((D, H), F32), pltpu.VMEM((256, 128), jnp.int32),
                        pltpu.VMEM((3, ROWS, H), BF), pltpu.VMEM((3, ROWS, H), BF),
                        pltpu.SemaphoreType.DMA((8,)), pltpu.SemaphoreType.DMA((3,)), pltpu.SemaphoreType.DMA((3,))],
        compiler_params=pltpu.CompilerParams(collective_id=0),
    )(x, router_W.T, route_idx.reshape(1, 256), expert_W, shared_W)
```

```python
import jax
import jax.numpy as jnp
from jax import lax
from jax.experimental import pallas as pl
from jax.experimental.pallas import tpu as pltpu

N_DEV = 4
ROWS = 64
HALF = 32
D = 128
H = 256
BF = jnp.bfloat16
F32 = jnp.float32
I32 = jnp.int32
MESH = pl.DeviceIdType.MESH
SIZES = ((2, -1, 16), (3, 16, 24), (4, 24, 32), (8, 32, 64))
EARLY_BAR = True
CP = dict(disable_bounds_checks=True, disable_semaphore_checks=True)


def dot(a, b):
    return jnp.dot(a, b, preferred_element_type=F32)


def onehot(m):
    return jnp.where(m, 1.0, 0.0).astype(BF)


def pallas_dist_moe_shared_ep_outshard_n256_d128_e2_h256_kernel(x, router_W, route_idx, expert_W, shared_W):
    def body(x_hbm, rw_hbm, idx_hbm, ew_hbm, sw_hbm, out_ref,
             x_v, rw_v, idx_v, ew_v, sw_v, send_buf, recv_buf, ld_sems, send_sems, recv_sems):
        ld_idx = pltpu.make_async_copy(idx_hbm, idx_v, ld_sems.at[0])
        ld_ew = [pltpu.make_async_copy(ew_hbm.at[j], ew_v.at[j], ld_sems.at[1 + j]) for j in range(2)]
        ld_idx.start(); ld_ew[0].start()
        me = lax.axis_index("i")
        blk = [(me + k) & 3 for k in range(N_DEV)]
        rows = [pl.ds(pl.multiple_of(b * ROWS, ROWS), ROWS) for b in blk]
        ld_x = [pltpu.make_async_copy(x_hbm.at[rows[k]], x_v.at[k], ld_sems.at[3 + k]) for k in range(N_DEV)]
        ld_rw = pltpu.make_async_copy(rw_hbm, rw_v, ld_sems.at[7])
        ld_sw = pltpu.make_async_copy(sw_hbm, sw_v, ld_sems.at[8])
        ld_x[2].start(); ld_ew[1].start()
        bar = pltpu.get_barrier_semaphore()
        for k in (2, 1, 3):
            pl.semaphore_signal(bar, inc=1, device_id=(blk[k],), device_id_type=MESH)
        ld_x[1].start(); ld_x[3].start(); ld_x[0].start(); ld_rw.start(); ld_sw.start()

        upper = onehot(lax.broadcasted_iota(I32, (128, 128), 0) < lax.broadcasted_iota(I32, (128, 128), 1))
        lane8 = lax.broadcasted_iota(I32, (8, 128), 1)
        sub8 = lax.broadcasted_iota(I32, (8, 128), 0)
        slot_h = lax.broadcasted_iota(I32, (HALF, 128), 0)

        ld_idx.wait()
        e_all = idx_v[...] & 7
        e_lo = jnp.broadcast_to(e_all[:, :128], (8, 128))
        e_hi = jnp.broadcast_to(e_all[:, 128:], (8, 128))
        b_s = jnp.where(sub8 < 4, (me + sub8) & 3, me)
        o_s = jnp.where(sub8 < 4, me, (me - sub8) & 3)
        e_s = jnp.where(b_s < 2, e_lo, e_hi)
        in_blk = (lane8 >> 6) == (b_s & 1)
        hit0 = in_blk & (e_s == 2 * o_s)
        hit1 = in_blk & (e_s == 2 * o_s + 1)
        h0 = jnp.where(hit0, 1.0, 0.0)
        h1 = jnp.where(hit1, 1.0, 0.0)
        n0_f = jnp.sum(h0, axis=1, keepdims=True)
        n_f = jnp.sum(h0 + h1, axis=1, keepdims=True)
        pre = dot(jnp.concatenate([h0, h1], axis=0).astype(BF), upper)
        pos = jnp.where(hit0, pre[:8], jnp.where(hit1, pre[8:] + n0_f, -1.0)).astype(I32)
        n0 = jnp.broadcast_to(n0_f, (8, 128)).astype(I32)
        n_i = jnp.broadcast_to(n_f, (8, 128)).astype(I32)
        cnt = {s: n_i[s, 0] for s in (2, 1, 3, 5, 6, 7)}

        def for_size(n, fn):
            for t, lo, hi in SIZES:
                pl.when((n > lo) & (n <= hi))(lambda t=t: fn(t))

        def rdma(k, t):
            s = pl.ds(0, 16 * t)
            return pltpu.make_async_remote_copy(send_buf.at[k - 1, s], recv_buf.at[k - 1, s], send_sems.at[k - 1], recv_sems.at[k - 1],
                                                device_id=(blk[k],), device_id_type=MESH)

        def gather(k, part):
            xb = x_v[k]
            return dot(onehot(slot_h + HALF * part == pos[k:k + 1, :]), jnp.concatenate([xb, xb], axis=0).astype(BF))

        def experts(xc):
            xc = xc.astype(BF)
            return [dot(xc, ew_v[j].astype(BF)) for j in range(2)]

        def store(k, part, y0, y1):
            first = slot_h + HALF * part < n0[k:k + 1, :]
            y = [jnp.where(first, y0[:, 128 * h:128 * h + 128], y1[:, 128 * h:128 * h + 128]) for h in range(2)]
            send_buf[k - 1, pl.ds(2 * HALF * part, 2 * HALF)] = jnp.concatenate(
                [y[h][8 * t:8 * t + 8] for t in range(HALF // 8) for h in range(2)], axis=0).astype(BF)

        def overflow(k):
            @pl.when(cnt[k] > HALF)
            def _():
                store(k, 1, *experts(gather(k, 1)))

        ld_ew[0].wait()
        ld_x[2].wait()
        xc = gather(2, 0)
        if EARLY_BAR:
            pl.semaphore_wait(bar, 3)
        ld_ew[1].wait()
        overflow(2)
        store(2, 0, *experts(xc))
        if not EARLY_BAR:
            pl.semaphore_wait(bar, 3)
        for_size(cnt[2], lambda t: rdma(2, t).start())

        ld_x[1].wait(); ld_x[3].wait()
        overflow(1); overflow(3)
        y0, y1 = experts(jnp.concatenate([gather(1, 0), gather(3, 0)], axis=0))
        store(1, 0, y0[:HALF], y1[:HALF])
        store(3, 0, y0[HALF:], y1[HALF:])
        for_size(cnt[1], lambda t: rdma(1, t).start())
        for_size(cnt[3], lambda t: rdma(3, t).start())

        ld_x[0].wait(); ld_rw.wait(); ld_sw.wait()
        xm = x_v[0]
        x2 = jnp.concatenate([xm, xm], axis=0)
        x_hi = x2.astype(BF)
        x_lo = (x2 - x_hi.astype(F32)).astype(BF)
        rw = rw_v[...]
        rw_hi = rw.astype(BF).astype(F32)
        rw2 = jnp.concatenate([rw_hi, rw - rw_hi], axis=0).astype(BF)
        nt = (((1,), (1,)), ((), ()))
        s2 = lax.dot_general(rw2, x_hi, nt, preferred_element_type=F32) + lax.dot_general(rw2, x_lo, nt, preferred_element_type=F32)
        scores = s2[:8] + s2[8:]
        pe = jnp.exp(scores - jnp.max(scores, axis=0, keepdims=True))
        e_row = e_s[4:5]
        p_row = jnp.sum(jnp.where(sub8 == e_row, pe, 0.0), axis=0, keepdims=True) / jnp.sum(pe, axis=0, keepdims=True)
        slot = jnp.max(jnp.where(sub8 >= 4, pos, -1).astype(F32), axis=0, keepdims=True).astype(I32)

        def to_col(row):
            t = jnp.broadcast_to(row, (128, 128)).T
            return jnp.where((me & 1) == 0, t[:ROWS], t[ROWS:])

        p = to_col(p_row)
        code = to_col((slot << 3) | e_row)
        e = code & 7
        slot_c = code >> 3
        col = ((slot_c >> 3) << 4) | (slot_c & 7)

        y0, y1 = experts(xm)
        sh = dot(xm.astype(BF), sw_v[...].astype(BF))
        acc = [sh[:, 128 * h:128 * h + 128] + p * jnp.where(e == 2 * me, y0[:, 128 * h:128 * h + 128], jnp.where(e == 2 * me + 1, y1[:, 128 * h:128 * h + 128], 0.0))
               for h in range(2)]

        lane_h = lax.broadcasted_iota(I32, (HALF, 2 * HALF), 1)
        row_r = lax.broadcasted_iota(I32, (2 * HALF, 128), 0)
        tok_r = ((row_r >> 4) << 3) | (row_r & 7)

        def scatter(k, part):
            c = jnp.where((e >> 1) == ((me - k) & 3), col - 2 * HALF * part, -16)[:, :2 * HALF]
            r = recv_buf[k - 1, pl.ds(2 * HALF * part, 2 * HALF)]
            r = jnp.where(tok_r + HALF * part < cnt[4 + k], r.astype(F32), 0.0).astype(BF)
            return [jnp.concatenate([dot(onehot(lane_h == c[HALF * g:HALF * g + HALF] + 8 * h), r) for g in range(2)], axis=0) for h in range(2)]

        for k in (1, 3):
            for_size(cnt[4 + k], lambda t, k=k: rdma(k, t).wait_recv())
        z1, z3 = scatter(1, 0), scatter(3, 0)
        acc = [acc[h] + p * (z1[h] + z3[h]) for h in range(2)]
        for k in (2, 1, 3):
            for_size(cnt[k], lambda t, k=k: rdma(k, t).wait_send())
        for_size(cnt[6], lambda t: rdma(2, t).wait_recv())
        z = scatter(2, 0)
        for h in range(2):
            out_ref[:, 128 * h:128 * h + 128] = acc[h] + p * z[h]
        for k in (1, 2, 3):
            @pl.when(cnt[4 + k] > HALF)
            def _(k=k):
                z = scatter(k, 1)
                for h in range(2):
                    out_ref[:, 128 * h:128 * h + 128] += p * z[h]

    hbm = pl.BlockSpec(memory_space=pltpu.HBM)
    return pl.pallas_call(
        body,
        out_shape=jax.ShapeDtypeStruct((ROWS, H), F32),
        in_specs=[hbm] * 5, out_specs=pl.BlockSpec(memory_space=pltpu.VMEM),
        scratch_shapes=[pltpu.VMEM((N_DEV, ROWS, D), F32), pltpu.VMEM((8, D), F32), pltpu.VMEM((1, 256), I32),
                        pltpu.VMEM((2, D, H), F32), pltpu.VMEM((D, H), F32),
                        pltpu.VMEM((3, 128, 128), BF), pltpu.VMEM((3, 128, 128), BF),
                        pltpu.SemaphoreType.DMA((9,)), pltpu.SemaphoreType.DMA((3,)), pltpu.SemaphoreType.DMA((3,))],
        compiler_params=pltpu.CompilerParams(collective_id=0, **CP),
    )(x, router_W.T, route_idx.reshape(1, 256), expert_W, shared_W)
```

```python
import jax
import jax.numpy as jnp
from jax import lax
from jax.experimental import pallas as pl
from jax.experimental.pallas import tpu as pltpu

N_DEV = 4
N_TOK = 256
N_EXP = 8
ROWS = 64
PART = 32
D = 128
H = 256
LANES = 128
NEAR, FAR = (1, 3), 2
NEAR_SIZES = (16, 24, PART, ROWS)
FAR_SIZES = (12, 16, 20, 24, PART, ROWS)

BF16 = jnp.bfloat16
F32 = jnp.float32
I32 = jnp.int32


def _dot(a, b):
    return jnp.dot(a, b, preferred_element_type=F32)


def _dot_nt(a, b):
    return lax.dot_general(a, b, (((1,), (1,)), ((), ())), preferred_element_type=F32)


def _onehot(mask):
    return jnp.where(mask, 1.0, 0.0).astype(BF16)


def _for_size(sizes, n, fn):
    lo = -1
    for hi in sizes:
        pl.when((n > lo) & (n <= hi))(lambda hi=hi: fn(hi))
        lo = hi


def _body(
    x_hbm, rw_hbm, idx_hbm, ew_hbm, sw_hbm, out_ref,
    x_v, rw_v, idx_v, ew_v, sw_v, send_buf, recv_buf, ld_sems, send_sems, recv_sems,
):
    cols = [pl.ds(LANES * h, LANES) for h in range(2)]

    ld_idx = pltpu.make_async_copy(idx_hbm, idx_v, ld_sems.at[0])
    ld_idx.start()
    me = lax.axis_index("i")

    def start_load_x(k):
        first = pl.multiple_of(((me + k) & 3) * ROWS, ROWS)
        copy = pltpu.make_async_copy(
            x_hbm.at[pl.ds(first, ROWS)], x_v.at[k], ld_sems.at[3 + k]
        )
        copy.start()
        return copy

    ld_x = {FAR: start_load_x(FAR)}
    ld_ew = [
        pltpu.make_async_copy(ew_hbm.at[:, :, cols[h]], ew_v.at[h], ld_sems.at[1 + h])
        for h in range(2)
    ]
    for copy in ld_ew:
        copy.start()
    peer = {k: (me + k) & 3 for k in (FAR, *NEAR)}
    barrier = pltpu.get_barrier_semaphore()
    for k in (FAR, *NEAR):
        pl.semaphore_signal(
            barrier, inc=1, device_id=(peer[k],), device_id_type=pl.DeviceIdType.MESH
        )
    for k in (*NEAR, 0):
        ld_x[k] = start_load_x(k)
    ld_rw = pltpu.make_async_copy(rw_hbm, rw_v, ld_sems.at[7])
    ld_sw = pltpu.make_async_copy(sw_hbm, sw_v, ld_sems.at[8])
    ld_rw.start()
    ld_sw.start()

    strict_upper = _onehot(
        lax.broadcasted_iota(I32, (LANES, LANES), 0)
        < lax.broadcasted_iota(I32, (LANES, LANES), 1)
    )
    lane = lax.broadcasted_iota(I32, (8, LANES), 1)
    sub = lax.broadcasted_iota(I32, (8, LANES), 0)
    row = lax.broadcasted_iota(I32, (ROWS, LANES), 0)

    ld_idx.wait()
    route = idx_v[...] & (N_EXP - 1)
    block = jnp.where(sub < 4, (me + sub) & 3, me)
    owner = jnp.where(sub < 4, me, (me - sub) & 3)
    expert = jnp.where(
        block < 2,
        jnp.broadcast_to(route[:, :LANES], (8, LANES)),
        jnp.broadcast_to(route[:, LANES:], (8, LANES)),
    )
    hit = ((lane >> 6) == (block & 1)) & ((expert >> 1) == owner)
    hit_f = jnp.where(hit, 1.0, 0.0)
    slot = _dot(hit_f.astype(BF16), strict_upper).astype(I32)
    total = jnp.sum(hit_f, axis=1, keepdims=True)
    total = jnp.broadcast_to(total, (8, LANES)).astype(I32)
    n_send = {k: total[k, 0] for k in (FAR, *NEAR)}
    n_recv = {k: total[4 + k, 0] for k in (FAR, *NEAR)}
    pack_row = jnp.where(
        hit, ((slot >> 5) << 6) | ((expert & 1) << 5) | (slot & (PART - 1)), -1
    )

    def pack(k, part):
        xb = x_v[k]
        packed = _dot(
            _onehot(row + ROWS * part == pack_row[k : k + 1]),
            jnp.concatenate([xb, xb], axis=0).astype(BF16),
        )
        return packed[:PART], packed[PART:]

    def experts(xs, h):
        y = [_dot(xs[j].astype(BF16), ew_v[h, j].astype(BF16)) for j in range(2)]
        return y[0] + y[1]

    def second_part(k, halves):
        @pl.when(n_send[k] > PART)
        def _():
            xs = pack(k, 1)
            for h in halves:
                send_buf[k - 1, h, pl.ds(PART, PART)] = experts(xs, h).astype(BF16)

    def near_copy(k, rows):
        return pltpu.make_async_remote_copy(
            send_buf.at[k - 1, :, pl.ds(0, rows)],
            recv_buf.at[k - 1, :, pl.ds(0, rows)],
            send_sems.at[k],
            recv_sems.at[k],
            device_id=(peer[k],),
            device_id_type=pl.DeviceIdType.MESH,
        )

    def far_copy(h, rows):
        return pltpu.make_async_remote_copy(
            send_buf.at[FAR - 1, h, pl.ds(0, rows)],
            recv_buf.at[FAR - 1, h, pl.ds(0, rows)],
            send_sems.at[2 * h],
            recv_sems.at[2 * h],
            device_id=(peer[FAR],),
            device_id_type=pl.DeviceIdType.MESH,
        )

    eager = me == 2
    n_eager = jnp.where(eager, n_send[FAR], -1)
    n_lazy = jnp.where(eager, -1, n_send[FAR])

    ld_x[FAR].wait()
    xs = pack(FAR, 0)
    pl.when(eager)(lambda: pl.semaphore_wait(barrier, N_DEV - 1))
    for h in range(2):
        ld_ew[h].wait()
        second_part(FAR, (h,))
        send_buf[FAR - 1, h, pl.ds(0, PART)] = experts(xs, h).astype(BF16)
        _for_size(FAR_SIZES, n_eager, lambda r, h=h: far_copy(h, r).start())

    for k in NEAR:
        ld_x[k].wait()
    for k in NEAR:
        second_part(k, (0, 1))
    xs = [jnp.concatenate(both, axis=0) for both in zip(*(pack(k, 0) for k in NEAR))]
    for h in range(2):
        y = experts(xs, h)
        for i, k in enumerate(NEAR):
            send_buf[k - 1, h, pl.ds(0, PART)] = (
                y[PART * i : PART * (i + 1)].astype(BF16)
            )
    pl.when(jnp.logical_not(eager))(lambda: pl.semaphore_wait(barrier, N_DEV - 1))
    for k in NEAR:
        _for_size(NEAR_SIZES, n_send[k], lambda r, k=k: near_copy(k, r).start())
    for h in range(2):
        _for_size(FAR_SIZES, n_lazy, lambda r, h=h: far_copy(h, r).start())

    ld_x[0].wait()
    ld_rw.wait()
    ld_sw.wait()
    x = x_v[0]
    x2 = jnp.concatenate([x, x], axis=0)
    x_hi = x2.astype(BF16)
    x_lo = (x2 - x_hi.astype(F32)).astype(BF16)
    rw = rw_v[...]
    rw_hi = rw.astype(BF16).astype(F32)
    rw2 = jnp.concatenate([rw_hi, rw - rw_hi], axis=0).astype(BF16)
    scores = _dot_nt(rw2, x_hi) + _dot_nt(rw2, x_lo)
    scores = scores[:N_EXP] + scores[N_EXP:]
    weights = jnp.exp(scores - jnp.max(scores, axis=0, keepdims=True))
    my_expert = expert[4:5]
    chosen = jnp.sum(jnp.where(sub == my_expert, weights, 0.0), axis=0, keepdims=True)

    def per_row(per_lane):
        t = jnp.broadcast_to(per_lane, (LANES, LANES)).T
        return jnp.where((me & 1) == 0, t[:ROWS], t[ROWS:])

    prob = per_row(chosen / jnp.sum(weights, axis=0, keepdims=True))
    info = per_row(my_expert | (slot[5:6] << 8) | (slot[6:7] << 16) | (slot[7:8] << 24))
    e = info & (N_EXP - 1)

    shared = _dot(x.astype(BF16), sw_v[...].astype(BF16))
    local = [jnp.where(e == 2 * me + j, x, 0.0) for j in range(2)]
    acc = [
        shared[:, LANES * h : LANES * (h + 1)] + prob * experts(local, h)
        for h in range(2)
    ]

    def unpack(k, h):
        slots = (info >> (8 * k)) & 127
        got = jnp.where(row < n_recv[k], recv_buf[k - 1, h].astype(F32), 0.0)
        tiles = []
        for t in range(ROWS // 8):
            s = slots[8 * t : 8 * t + 8]
            base = jnp.broadcast_to(s[0:1], (8, LANES))
            src_tile = (base + ((sub - base) & 7)) >> 3
            window = got[0:8]
            for c in range(1, t + 1):
                window = jnp.where(src_tile == c, got[8 * c : 8 * c + 8], window)
            tiles.append(jnp.take_along_axis(window, s & 7, axis=0))
        scale = jnp.where((e >> 1) == ((me - k) & 3), prob, 0.0)
        return scale * jnp.concatenate(tiles, axis=0)

    for k in NEAR:
        _for_size(NEAR_SIZES, n_recv[k], lambda r, k=k: near_copy(k, r).wait_recv())
    for k in NEAR:
        acc = [acc[h] + unpack(k, h) for h in range(2)]
    for k in NEAR:
        _for_size(NEAR_SIZES, n_send[k], lambda r, k=k: near_copy(k, r).wait_send())
    for h in range(2):
        _for_size(FAR_SIZES, n_send[FAR], lambda r, h=h: far_copy(h, r).wait_send())
    for h in range(2):
        _for_size(FAR_SIZES, n_recv[FAR], lambda r, h=h: far_copy(h, r).wait_recv())
        out_ref[:, cols[h]] = acc[h] + unpack(FAR, h)


def pallas_dist_moe_shared_ep_outshard_n256_d128_e2_h256_kernel(
    x: jax.Array,
    router_W: jax.Array,
    route_idx: jax.Array,
    expert_W: jax.Array,
    shared_W: jax.Array,
):
    return pl.pallas_call(
        _body,
        out_shape=jax.ShapeDtypeStruct((ROWS, H), F32),
        in_specs=[pl.BlockSpec(memory_space=pltpu.HBM)] * 5,
        out_specs=pl.BlockSpec(memory_space=pltpu.VMEM),
        scratch_shapes=[
            pltpu.VMEM((N_DEV, ROWS, D), F32),
            pltpu.VMEM((N_EXP, D), F32),
            pltpu.VMEM((1, N_TOK), I32),
            pltpu.VMEM((2, 2, D, LANES), F32),
            pltpu.VMEM((D, H), F32),
            pltpu.VMEM((N_DEV - 1, 2, ROWS, LANES), BF16),
            pltpu.VMEM((N_DEV - 1, 2, ROWS, LANES), BF16),
            pltpu.SemaphoreType.DMA((9,)),
            pltpu.SemaphoreType.DMA((4,)),
            pltpu.SemaphoreType.DMA((4,)),
        ],
        compiler_params=pltpu.CompilerParams(
            collective_id=0, disable_semaphore_checks=True
        ),
    )(x, router_W.T, route_idx.reshape(1, N_TOK), expert_W, shared_W)
```
